```python
import numpy as np

kernel_name = "dist_sort_i_m128_n64"

def setup_inputs():
    return {"x": np.random.randn(512, 64).astype(np.float32)}

def reference(x: np.ndarray) -> np.ndarray:
    return np.sort(x, axis=0)
```

```python
import jax, jax.numpy as jnp
from jax import lax
from jax.experimental import pallas as pl
from jax.experimental.pallas import tpu as pltpu

NET16 = [
 [(0,13),(1,12),(2,15),(3,14),(4,8),(5,6),(7,11),(9,10)],
 [(0,5),(1,7),(2,9),(3,4),(6,13),(8,14),(10,15),(11,12)],
 [(0,1),(2,3),(4,5),(6,8),(7,9),(10,11),(12,13),(14,15)],
 [(0,2),(1,3),(4,10),(5,11),(6,7),(8,9),(12,14),(13,15)],
 [(1,2),(3,12),(4,6),(5,7),(8,10),(9,11),(13,14)],
 [(1,4),(2,6),(5,8),(7,10),(9,13),(11,14)],
 [(2,4),(3,6),(9,12),(11,13)],
 [(3,5),(6,8),(7,9),(10,12)],
 [(3,4),(5,6),(7,8),(9,10),(11,12)],
 [(6,7),(8,9)],
]

class Ops:
    def __init__(self, mn, mx, where, roll, masks):
        self.mn, self.mx, self.where, self.roll = mn, mx, where, roll
        self.m0 = masks
    def flipped(self):
        return Ops(self.mx, self.mn, self.where, self.roll, self.m0)

def up(o, x, d):
    return o.roll(x, d % 8)
def down(o, x, d):
    return o.roll(x, (-d) % 8)

def xorperm(o, x, mask):
    if mask == 4: return o.roll(x, 4)
    if mask == 6:
        return o.where(o.m0[1], up(o, x, 2), down(o, x, 2))
    raise NotImplementedError

def vstage(o, r, k):
    r = list(r); bit = 1 << k
    for v in range(len(r)):
        if not v & bit:
            a, b = r[v], r[v | bit]
            r[v], r[v | bit] = o.mn(a, b), o.mx(a, b)
    return r

def swapstage(o, r, j, k, neg=None):
    r = list(r); bit = 1 << k; d = 1 << j; m = o.m0[j]
    for v in range(len(r)):
        if not v & bit:
            a, b = r[v], r[v | bit]
            if j == 2 and neg is None:
                p = o.where(m, a, b); q = o.roll(o.where(m, b, a), 4)
            else:
                p = o.where(m, a, up(o, b, d)); q = o.where(m, down(o, a, d), b)
                if neg is not None: q = neg(q)
            r[v], r[v | bit] = o.mn(p, q), o.mx(p, q)
    return r

def mirrorstage(o, r, mask, k):
    out = list(r); bit = 1 << k; n = len(r)
    for v in range(n):
        if not v & bit:
            a, b = r[v], xorperm(o, r[(n - 1) ^ v], mask)
            out[v], out[v | bit] = o.mn(a, b), o.mx(a, b)
    return out

def dstage(o, r, j):
    d = 1 << j; m = o.m0[j]; out = []
    for a in r:
        if j == 2:
            t = o.roll(a, 4)
            out.append(o.where(m, o.mn(a, t), o.mx(a, t)))
        else:
            out.append(o.where(m, o.mn(a, down(o, a, d)), o.mx(a, up(o, a, d))))
    return out

def permute_slots(r, slots, order):
    out = [None] * len(r)
    for v in range(len(r)):
        w = 0
        for k, b in enumerate(slots):
            if v >> k & 1: w |= 1 << order.index(b)
        out[w] = r[v]
    return out

def sort128(o, r, neg):
    r = list(r)
    for layer in NET16:
        for a, b in layer:
            r[a], r[b] = o.mn(r[a], r[b]), o.mx(r[a], r[b])
    s = [0, 1, 2, 3]
    K = lambda b: s.index(b)
    def put(old, new): s[s.index(old)] = new
    r = mirrorstage(o, r, 4, K(0)); put(0, 4)
    for b in (3, 2, 1): r = vstage(o, r, K(b))
    r = swapstage(o, r, 2, K(1)); put(1, 0)
    r = mirrorstage(o, r, 6, K(0)); put(0, 5)
    for b in (4, 3, 2): r = vstage(o, r, K(b))
    r = swapstage(o, r, 2, K(2)); put(2, 1)
    r = swapstage(o, r, 1, K(1)); put(1, 0)
    r = swapstage(o, r, 0, K(0), neg=neg); put(0, 6)
    for b in (5, 4, 3): r = vstage(o, r, K(b))
    r = swapstage(o, r, 2, K(3)); put(3, 2)
    r = swapstage(o, r, 1, K(2)); put(2, 1)
    r = swapstage(o, r, 0, K(1)); put(1, 0)
    return permute_slots(r, s, [0, 4, 5, 6])

def merge7(o, r):
    for k in (3, 2, 1): r = vstage(o, r, k)
    for j in (2, 1, 0): r = dstage(o, r, j)
    return vstage(o, r, 0)


W = 64
NT = (((1,), (1,)), ((), ()))
MESH = pl.DeviceIdType.MESH

def make_ops():
    sub = lax.broadcasted_iota(jnp.int32, (8, W), 0)
    return Ops(jnp.minimum, jnp.maximum, jnp.where, lambda x, d: pltpu.roll(x, d, 0), [(sub >> j & 1) == 0 for j in range(3)])

def in_T(b, nsplit=2):
    out = []
    m = 128 // nsplit
    for h in range(nsplit):
        r = lax.broadcasted_iota(jnp.int32, (m, 128), 0) + h * m
        c = lax.broadcasted_iota(jnp.int32, (m, 128), 1)
        L = jnp.where(r == c, jnp.where(r & 1 == 1, -1.0, 1.0), 0.0).astype(jnp.bfloat16)
        t = lax.dot_general(L, b, NT, preferred_element_type=jnp.float32)
        out += [t[8 * v:8 * v + 8] for v in range(m // 8)]
    return out

def out_T(r, o_ref, nsplit=2):
    w = []
    for u in range(8):
        lo = pltpu.bitcast(r[2 * u], jnp.uint32); hi = pltpu.bitcast(r[2 * u + 1], jnp.uint32)
        w.append(pltpu.bitcast((lo >> 16) | hi, jnp.bfloat16))
    R = jnp.concatenate(w, axis=0)
    m = 64 // nsplit
    for h in range(nsplit):
        i = lax.broadcasted_iota(jnp.int32, (m, 64), 0) + h * m; j = lax.broadcasted_iota(jnp.int32, (m, 64), 1)
        L = jnp.where(i == j, 1.0, 0.0).astype(jnp.bfloat16)
        o_ref[h * m:(h + 1) * m, :] = lax.dot_general(L, R, NT, preferred_element_type=jnp.float32)

def pallas_dist_sort_i_m128_n64_kernel(x, compute=True):
    xt = x.T
    def body(x_ref, o_ref, xv, sbuf, rbuf, lsem, ssem, rsem, reg):
        me = lax.axis_index("i")
        bs = pltpu.get_barrier_semaphore()
        def sig(sem, dev): pl.semaphore_signal(sem, inc=1, device_id=(dev,), device_id_type=MESH)
        def slot(src, dst):
            return {1: 0, 3: 1, 2: 2}[(src - dst) % 4]
        def send(src, dst):
            s = slot(src, dst)
            pltpu.make_async_remote_copy(src_ref=sbuf, dst_ref=rbuf.at[s], send_sem=ssem.at[s], recv_sem=rsem.at[s],
                                         device_id=(dst,), device_id_type=MESH).start()
        def desc(s):
            return pltpu.make_async_remote_copy(src_ref=sbuf, dst_ref=rbuf.at[s], send_sem=ssem.at[s], recv_sem=rsem.at[s],
                                                device_id=(0,), device_id_type=MESH)
        cp = pltpu.make_async_copy(x_ref, xv, lsem)
        cp.start()
        @pl.when(me == 0)
        def _():
            sig(bs, 2); sig(bs, 1); sig(bs, 3)
        for k in (1, 3):
            @pl.when(me == k)
            def _():
                sig(bs, 2)
                pl.semaphore_wait(bs, 1)
                sig(reg.at[k // 2], 0)
        @pl.when(me == 2)
        def _():
            sig(bs, 0)
            pl.semaphore_wait(bs, 3)
            sig(reg.at[0], 1); sig(reg.at[0], 3)
        cp.wait()
        xb = xv[...].astype(jnp.bfloat16)
        sbuf[...] = xb
        for k in (1, 3):
            @pl.when(me == k)
            def _():
                send(k, 0)
        @pl.when(me == 2)
        def _():
            send(2, 0); send(2, 3); send(2, 1)
        o = make_ops(); neg = lambda q: -q
        if compute:
            A = sort128(o, in_T(xb), neg)
        @pl.when(me == 0)
        def _():
            pl.semaphore_wait(reg.at[0], 1); send(0, 1)
            pl.semaphore_wait(reg.at[1], 1); send(0, 3)
            pl.semaphore_wait(bs, 1); send(0, 2)
        for k in (1, 3):
            @pl.when(me == k)
            def _():
                pl.semaphore_wait(reg.at[0], 1)
                send(k, k ^ 2); send(k, 2)
        desc(0).wait_recv()
        if compute:
            X = sort128(o.flipped(), in_T(rbuf[0]), neg)
            M0 = merge7(o, [jnp.minimum(p, q) for p, q in zip(A, X)])
            M1 = merge7(o, [jnp.maximum(p, q) for p, q in zip(A, X)])
            inf = jnp.full((8, W), jnp.inf, jnp.float32)
            def pick(j):
                return [jnp.where(j < 0, -inf, jnp.where(j == 0, a, jnp.where(j == 1, b, inf))) for a, b in zip(M0, M1)]
            Ba, Bb, Bc = pick(me - 2), pick(me - 1), pick(me)
        desc(1).wait_recv()
        cl = lambda y, lo, hi: [jnp.maximum(l, jnp.minimum(t, h)) for t, l, h in zip(y, lo, hi)]
        if compute:
            Y = sort128(o.flipped(), in_T(rbuf[1]), neg)
            Slo = merge7(o, cl(Y, Ba, Bb)); Shi = merge7(o, cl(Y, Bb, Bc))
        desc(2).wait_recv()
        if compute:
            D = sort128(o.flipped(), in_T(rbuf[2]), neg)
            R = merge7(o, cl(D, Slo, Shi))
            out_T(R, o_ref)
        else:
            o_ref[...] = (rbuf[0] + rbuf[1] + rbuf[2]).astype(jnp.float32)
        for s in range(3):
            desc(s).wait_send()
    return pl.pallas_call(body, out_shape=jax.ShapeDtypeStruct(xt.shape, xt.dtype),
        in_specs=[pl.BlockSpec(memory_space=pl.ANY)], out_specs=pl.BlockSpec(memory_space=pltpu.VMEM),
        scratch_shapes=[pltpu.VMEM((64, 128), jnp.float32), pltpu.VMEM((64, 128), jnp.bfloat16),
                        pltpu.VMEM((3, 64, 128), jnp.bfloat16),
                        pltpu.SemaphoreType.DMA, pltpu.SemaphoreType.DMA((3,)), pltpu.SemaphoreType.DMA((3,)),
                        pltpu.SemaphoreType.REGULAR((2,))],
        compiler_params=pltpu.CompilerParams(collective_id=0, disable_bounds_checks=True, disable_semaphore_checks=True))(xt).T
```

```python
import functools

import jax
import jax.numpy as jnp
from jax import lax
from jax.experimental import pallas as pl
from jax.experimental.pallas import tpu as pltpu

BF, F32, U32 = jnp.bfloat16, jnp.float32, jnp.uint32
MESH = pl.DeviceIdType.MESH
NT = (((1,), (1,)), ((), ()))

COLS = 64
RAW = 24
NB = COLS - RAW
EARLY = 16
MXU_BLOCKS = (2, 2, 3, 3)
XLU_SPLITS = ((2, 32), (3, 64))

NET16 = (
    (0, 13), (1, 12), (2, 15), (3, 14), (4, 8), (5, 6), (7, 11), (9, 10),
    (0, 5), (1, 7), (2, 9), (3, 4), (6, 13), (8, 14), (10, 15), (11, 12),
    (0, 1), (2, 3), (4, 5), (6, 8), (7, 9), (10, 11), (12, 13), (14, 15),
    (0, 2), (1, 3), (4, 10), (5, 11), (6, 7), (8, 9), (12, 14), (13, 15),
    (1, 2), (3, 12), (4, 6), (5, 7), (8, 10), (9, 11), (13, 14),
    (1, 4), (2, 6), (5, 8), (7, 10), (9, 13), (11, 14),
    (2, 4), (3, 6), (9, 12), (11, 13),
    (3, 5), (6, 8), (7, 9), (10, 12),
    (3, 4), (5, 6), (7, 8), (9, 10), (11, 12),
    (6, 7), (8, 9),
)
WIRE = (0, 1, 3, 2, 10, 8, 12, 9, 14, 11, 15, 13, 5, 4, 6, 7)

LAYOUT_G = (2, 1, 3)
LAYOUT_F = (3, 2, 1)
VREG_BITS = (0, 4, 5, 6)


def _roll(x, d):
    return pltpu.roll(x, d % 8, 0)


def _pack(lo, hi):
    return (pltpu.bitcast(lo, U32) >> 16) | pltpu.bitcast(hi, U32)


class _Net:
    def __init__(self, regs, vbits, sbits, ascending):
        self.r, self.vb, self.sb, self.asc = list(regs), list(vbits), list(sbits), ascending
        sub = lax.broadcasted_iota(jnp.int32, (8, COLS), 0)
        self.low = [(sub >> j) & 1 == 0 for j in range(3)]

    def cx(self, a, b, skew=False):
        if skew:
            c = ((a < b) if self.asc else (b < a)) != self.low[2]
            return jnp.where(c, b, a), jnp.where(c, a, b)
        lo, hi = jnp.minimum(a, b), jnp.maximum(a, b)
        return (lo, hi) if self.asc else (hi, lo)

    def _pairs(self, bit, fn):
        k = 1 << self.vb.index(bit)
        old = list(self.r)
        for v in range(16):
            if not v & k:
                self.r[v], self.r[v | k] = fn(old, v, v | k)

    def _trade(self, bit, evict):
        self.vb[self.vb.index(evict)] = bit
        self.sb[self.sb.index(bit)] = evict

    def stage(self, *bits, skew=False):
        for b in bits:
            self._pairs(b, lambda r, v, w: self.cx(r[v], r[w], skew))

    def swap(self, bit, evict, negate=False, skew=False):
        j = 2 - self.sb.index(bit)
        d, m = 1 << j, self.low[j]

        def fn(r, v, w):
            p = jnp.where(m, r[v], _roll(r[w], d))
            q = jnp.where(m, _roll(r[v], -d), r[w])
            return self.cx(p, -q if negate else q, skew)

        self._pairs(evict, fn)
        self._trade(bit, evict)

    def rot4(self, bit, evict):
        assert self.sb[0] == bit
        self._pairs(evict, lambda r, v, w: self.cx(r[v], _roll(r[w], 4)))
        self._trade(bit, evict)

    def mirror(self, bit, evict):
        mask = sum(4 >> t for t in range(3) if self.sb[t] <= bit)

        def flip(x):
            if mask == 4:
                return _roll(x, 4)
            assert mask == 6
            return jnp.where(self.low[1], _roll(x, 2), _roll(x, -2))

        self._pairs(evict, lambda r, v, w: self.cx(r[v], flip(r[15 ^ v])))
        self._trade(bit, evict)

    def shuffle(self, evict):
        def fn(r, v, w):
            t = pltpu.bitcast(_pack(r[v], r[w]), BF).astype(F32)
            return t[:8], t[8:]

        self._pairs(evict, fn)
        self.vb[self.vb.index(evict)] = self.sb[0]
        self.sb = [self.sb[1], self.sb[2], evict]

    def result(self, sbits):
        assert tuple(self.sb) == sbits
        out = [None] * 16
        for v in range(16):
            out[sum(((v >> k) & 1) << VREG_BITS.index(b) for k, b in enumerate(self.vb))] = self.r[v]
        return out


def _sort(t, ascending):
    n = _Net([t[i] for i in WIRE], (0, 1, 2, 3), (4, 5, 6), ascending)
    for a, b in NET16:
        n.r[a], n.r[b] = n.cx(n.r[a], n.r[b])
    n.mirror(4, 0); n.stage(3, 2); n.stage(1, skew=True); n.rot4(0, 1)
    n.mirror(5, 0); n.stage(4, 3, 2); n.shuffle(2); n.stage(1, skew=True); n.rot4(0, 1)
    n.swap(6, 0, negate=True); n.stage(5, 4, 3); n.swap(2, 3, skew=True); n.rot4(1, 2); n.swap(0, 1)
    return n.result(LAYOUT_G)


def _merge(r, final=False):
    n = _Net(r, VREG_BITS, LAYOUT_G, True)
    n.stage(6, 5, 4)
    if final:
        n.swap(3, 0, skew=True); n.rot4(2, 3); n.swap(1, 2); n.swap(0, 1)
        return n.result(LAYOUT_F)
    n.swap(3, 0); n.shuffle(3); n.stage(2, skew=True); n.rot4(1, 2); n.swap(0, 1)
    return n.result(LAYOUT_G)


def _clamp(y, lo, hi):
    return [jnp.maximum(l, jnp.minimum(t, h)) for t, l, h in zip(y, lo, hi)]


def _load(ref):
    return [ref[8 * v:8 * v + 8] for v in range(16)]


def _store(ref, regs):
    for v in range(16):
        ref[8 * v:8 * v + 8] = regs[v]


def _init_identities(eye_in, eye_out):
    r = lax.broadcasted_iota(jnp.int32, (128, 128), 0)
    c = lax.broadcasted_iota(jnp.int32, (128, 128), 1)
    sign = jnp.where(r & 1 == 1, -1.0, 1.0)
    eye_in[...] = pltpu.bitcast(jnp.where(r == c, sign, 0.0).astype(BF), U32)
    r = lax.broadcasted_iota(jnp.int32, (COLS, COLS), 0)
    c = lax.broadcasted_iota(jnp.int32, (COLS, COLS), 1)
    eye_out[...] = pltpu.bitcast(jnp.where(r == c, 1.0, 0.0).astype(BF), U32)


def _transpose_in(b, eye_in, assist=False):
    eye = [pltpu.bitcast(eye_in[8 * g:8 * g + 8, :], BF) for g in range(8)]
    lhs = [eye[2 * h:2 * h + 2] for h in range(4)]
    extra = [[]] * 4
    if assist:
        lhs = [eye[1:3], eye[3:5], [eye[5], eye[6][:8]], [eye[7], eye[6][8:]]]
        t = pltpu.bitcast(b[:, :16].T, U32) ^ jnp.uint32(0x80000000)
        t = pltpu.bitcast(t, BF).astype(F32)
        extra = [[], [], [t[:8]], [t[8:]]]
    out = []
    for h in range(4):
        t = lax.dot_general(jnp.concatenate(lhs[h], axis=0), b, NT, preferred_element_type=F32)
        out += [t[v:v + 8] for v in range(0, t.shape[0], 8)] + extra[h]
    return out


def _transpose_out(r, eye_out, o_ref):
    w = [_pack(r[2 * u], r[2 * u + 1]) for u in range(8)]
    zero = jnp.zeros((8, COLS), U32)
    hi = {}
    for k, ncols in XLU_SPLITS:
        t = pltpu.bitcast(jnp.concatenate([zero] * k + w[k:], axis=0), BF)
        hi[k] = t[:, :ncols].T.astype(F32)

    def store_hi(h):
        k = MXU_BLOCKS[h]
        o_ref[16 * h:16 * h + 16, 16 * k:] = hi[k][16 * h:16 * h + 16, 16 * k:]

    for h in range(3):
        store_hi(h)
    for h in (3, 2, 1, 0):
        k = MXU_BLOCKS[h]
        lo = pltpu.bitcast(jnp.concatenate(w[:k], axis=0), BF)
        eye = pltpu.bitcast(eye_out[8 * h:8 * h + 8, :], BF)
        o_ref[16 * h:16 * h + 16, :16 * k] = lax.dot_general(eye, lo, NT, preferred_element_type=F32)
    store_hi(3)


CHUNKS = tuple((8 * i, 8) for i in range(NB // 8)) + ((NB, RAW),)
FIRST, SECOND, LAST = 0, 1, 2
N_CHUNKS = len(CHUNKS)
FWD = 3


def _body(x_ref, o_ref, xv, sbuf, rbuf, rawbuf, eye_in, eye_out, s_list, s_m, s_s,
          lsem, ssem, rsem, ack):
    barrier = pltpu.get_barrier_semaphore()
    me = lax.axis_index("i")

    def signal(sem, dev):
        pl.semaphore_signal(sem, inc=1, device_id=(dev,), device_id_type=MESH)

    def rows(ref, lo, n):
        return ref.at[pl.ds(lo, n)]

    def rdma(src, dst, s, r, dev=0):
        return pltpu.make_async_remote_copy(
            src_ref=src, dst_ref=dst, send_sem=ssem.at[s], recv_sem=rsem.at[r],
            device_id=(dev,), device_id_type=MESH)

    def shard(slot, s, dev=0, lo=0, n=COLS):
        return rdma(rows(sbuf, lo, n), rows(rbuf.at[slot], lo, n), s, slot, dev)

    def chunk(src, i, s, dev=0):
        return rdma(rows(src, *CHUNKS[i]), rows(rbuf.at[LAST], *CHUNKS[i]), s, LAST + i, dev)

    def raw():
        return rdma(rows(x_ref, NB, RAW), rawbuf, 0, LAST + N_CHUNKS - 1, 0)

    def load(i):
        return pltpu.make_async_copy(rows(x_ref, *CHUNKS[i]), rows(xv, *CHUNKS[i]), lsem.at[i])

    load(0).start()

    @pl.when(me == 2)
    def _():
        signal(barrier, 0)
        pl.semaphore_wait(barrier, 1)
        raw().start()

    for i in range(1, N_CHUNKS - 1):
        load(i).start()

    @pl.when(me != 2)
    def _():
        load(N_CHUNKS - 1).start()

    @pl.when(me == 0)
    def _():
        for dev in (2, 1, 3):
            signal(barrier, dev)

    for k in (1, 3):
        @pl.when(me == k)
        def _():
            pl.semaphore_wait(barrier, 1)
            signal(ack.at[k // 2], 0)

    _init_identities(eye_in, eye_out)

    sent = 0
    for i, (lo, n) in enumerate(CHUNKS):
        load(i).wait()
        sbuf[lo:lo + n] = xv[lo:lo + n].astype(BF)
        if i < N_CHUNKS - 1:
            @pl.when(me == 2)
            def _():
                chunk(sbuf, i, 1).start()
                if i == 0:
                    load(N_CHUNKS - 1).start()
        if lo + n in (EARLY, COLS):
            for k in (1, 3):
                @pl.when(me == k)
                def _():
                    shard(k // 2, 0, 0, sent, lo + n - sent).start()
            sent = lo + n

    _store(s_list, _sort(_transpose_in(sbuf[...], eye_in), True))
    inf = jnp.full((128, COLS), jnp.inf, F32)
    s_m[0] = -inf
    s_m[3] = inf
    s_s[0] = -inf
    s_s[1] = inf

    @pl.when(me == 0)
    def _():
        pl.semaphore_wait(ack.at[0], 1)
        shard(FIRST, 0, 1).start()
        pl.semaphore_wait(ack.at[1], 1)
        shard(FIRST, 1, 3).start()
        signal(ack.at[0], 1)
        signal(ack.at[0], 3)
        pl.semaphore_wait(barrier, 1)
        shard(FIRST, 2, 2).start()
        signal(ack.at[1], 1)

    for k in (1, 3):
        @pl.when(me == k)
        def _():
            pl.semaphore_wait(ack.at[0], 1)
            shard(SECOND, 1, k ^ 2).start()
            if k == 1:
                pl.semaphore_wait(ack.at[1], 1)
                shard(SECOND, 2, 2).start()

    shard(FIRST, 0).wait_recv()

    @pl.when(me == 0)
    def _():
        signal(ack.at[1], 3)

    @pl.when(me == 3)
    def _():
        pl.semaphore_wait(ack.at[1], 1)
        for i in range(N_CHUNKS):
            chunk(sbuf, i, 2, 2).start()

    shard(SECOND, 0).wait_recv()
    t1 = _transpose_in(rbuf[FIRST], eye_in)
    t2 = _transpose_in(rbuf[SECOND], eye_in)
    first = _sort(t1, False)
    own = _load(s_list)
    _store(s_m.at[1], [jnp.minimum(a, b) for a, b in zip(own, first)])
    _store(s_m.at[2], [jnp.maximum(a, b) for a, b in zip(own, first)])
    _store(s_list, _sort(t2, False))

    @pl.when(me < 3)
    def _():
        _store(s_m.at[1], _merge(_load(s_m.at[1])))

    @pl.when(me > 0)
    def _():
        _store(s_m.at[2], _merge(_load(s_m.at[2])))

    @pl.when(me > 0)
    def _():
        _store(s_s.at[0], _merge(_clamp(_load(s_list), _load(s_m.at[me - 1]), _load(s_m.at[me]))))

    @pl.when(me < 3)
    def _():
        _store(s_s.at[1], _merge(_clamp(_load(s_list), _load(s_m.at[me]), _load(s_m.at[me + 1]))))

    @pl.when(me != 2)
    def _():
        for s in range(3):
            shard(FIRST, s).wait_send()

    @pl.when(me == 2)
    def _():
        raw().wait_send()
        shard(FIRST, 1, n=NB).wait_send()

    def forward(i):
        for dev in (1, 3):
            chunk(rbuf.at[LAST], i, FWD, dev).start()

    @pl.when(me == 0)
    def _():
        raw().wait_recv()
        rbuf[LAST, NB:COLS] = rawbuf[...].astype(BF)
        forward(N_CHUNKS - 1)

    @pl.when(me != 0)
    def _():
        chunk(sbuf, N_CHUNKS - 1, 0).wait_recv()

    tail = (NB - 8) // 16 * 16
    for i in range(N_CHUNKS - 1):
        if i == N_CHUNKS - 2:
            below = pltpu.bitcast(rbuf[LAST, 0:tail], U32)
            above = pltpu.bitcast(rbuf[LAST, tail + 16:COLS], U32)
        chunk(sbuf, i, 0).wait_recv()
        pl.when(me == 0)(functools.partial(forward, i))

    mid = pltpu.bitcast(rbuf[LAST, tail:tail + 16], U32)
    last = pltpu.bitcast(jnp.concatenate([below, mid, above], axis=0), BF)
    last = _sort(_transpose_in(last, eye_in, assist=True), False)
    quarter = _merge(_clamp(last, _load(s_s.at[0]), _load(s_s.at[1])), final=True)
    _transpose_out(quarter, eye_out, o_ref)

    @pl.when(me == 0)
    def _():
        two = rbuf.at[pl.ds(0, 2)]
        rdma(two, two, FWD, 0).wait_send()


def pallas_dist_sort_i_m128_n64_kernel(x: jax.Array):
    xt = x.T
    out = pl.pallas_call(
        _body,
        out_shape=jax.ShapeDtypeStruct(xt.shape, xt.dtype),
        in_specs=[pl.BlockSpec(memory_space=pl.ANY)],
        out_specs=pl.BlockSpec(memory_space=pltpu.VMEM),
        scratch_shapes=[
            pltpu.VMEM((COLS, 128), F32),
            pltpu.VMEM((COLS, 128), BF),
            pltpu.VMEM((3, COLS, 128), BF),
            pltpu.VMEM((RAW, 128), F32),
            pltpu.VMEM((64, 128), U32),
            pltpu.VMEM((COLS // 2, COLS), U32),
            pltpu.VMEM((128, COLS), F32),
            pltpu.VMEM((4, 128, COLS), F32),
            pltpu.VMEM((2, 128, COLS), F32),
            pltpu.SemaphoreType.DMA((N_CHUNKS,)),
            pltpu.SemaphoreType.DMA((4,)),
            pltpu.SemaphoreType.DMA((LAST + N_CHUNKS,)),
            pltpu.SemaphoreType.REGULAR((2,)),
        ],
        compiler_params=pltpu.CompilerParams(
            collective_id=0,
            disable_bounds_checks=True,
            disable_semaphore_checks=True,
        ),
    )(xt)
    return out.T
```
